```python
import numpy as np

kernel_name = "dist_halo_stencil_i_m8192_n1024"

def setup_inputs():
    return {"x": np.random.randn(32768, 1024).astype(np.float32)}

def reference(x: np.ndarray) -> np.ndarray:
    out = np.empty_like(x)
    out[0] = x[0]
    out[-1] = x[-1]
    out[1:-1] = 0.25 * x[:-2] + 0.5 * x[1:-1] + 0.25 * x[2:]
    return out
```

```python
import jax
import jax.numpy as jnp
from jax import lax
from jax.experimental import pallas as pl
from jax.experimental.pallas import tpu as pltpu

M, N = 8192, 1024
NDEV = 4
P, Q, U = 4, 16, 16
G = P * Q
CT = N // 128
W = U * N

def make(nt=3, tw=1, compute=True, nodma=False, halo_at=30, ahead=4, comm="row", bar_at=2, sig=True, ring=True, dsc=False):
    NP = P * U - nt
    u0 = U - 1 - nt
    def body(x_hbm, y_ref, xb, sbuf, rbuf, msem, csem, ssem, hsem):
        me = lax.axis_index("i")
        left = lax.rem(me + NDEV - 1, NDEV)
        right = lax.rem(me + 1, NDEV)

        def piece(k):
            j = k - 1
            j = j + jnp.where(j >= (P - 1) * U, 1, 0)
            p = jnp.where(k == 0, P - 1, j >> 4)
            u = jnp.where(k == 0, U - 1, (j - 1) & (U - 1))
            return pltpu.make_async_copy(x_hbm.at[pl.ds(p * Q, Q), u], xb.at[pl.ds(1 + p * Q, Q), u], msem.at[k % ahead if ring else k])
        def cpiece(c):
            cols = pl.ds(c * (128 * tw) if isinstance(c, int) else pl.multiple_of(c * (128 * tw), 128), 128 * tw)
            return pltpu.make_async_copy(x_hbm.at[pl.ds((P - 1) * Q, Q), pl.ds(u0, nt), :, cols],
                                         xb.at[pl.ds(1 + (P - 1) * Q, Q), pl.ds(u0, nt), :, cols], csem.at[c])
        def start(c):
            if not nodma: c.start()
        def wait(c):
            if not nodma: c.wait()

        for k in range(ahead):
            start(piece(k))
        if sig:
            bar = pltpu.get_barrier_semaphore()
            for n in (left, right):
                pl.semaphore_signal(bar, inc=1, device_id=(n,), device_id_type=pl.DeviceIdType.MESH)
        if comm == "band":
            to_left = pltpu.make_async_remote_copy(xb.at[1, 0], xb.at[G + 1, 0], ssem.at[0], hsem.at[1],
                                                   device_id=(left,), device_id_type=pl.DeviceIdType.MESH)
            to_right = pltpu.make_async_remote_copy(xb.at[G, U - 1], xb.at[0, U - 1], ssem.at[1], hsem.at[0],
                                                    device_id=(right,), device_id_type=pl.DeviceIdType.MESH)
        elif comm == "row":
            to_left = pltpu.make_async_remote_copy(sbuf.at[0], rbuf.at[1], ssem.at[0], hsem.at[1],
                                                   device_id=(left,), device_id_type=pl.DeviceIdType.MESH)
            to_right = pltpu.make_async_remote_copy(sbuf.at[1], rbuf.at[0], ssem.at[1], hsem.at[0],
                                                    device_id=(right,), device_id_type=pl.DeviceIdType.MESH)

        sub = lax.broadcasted_iota(jnp.int32, (Q, 8, 128), 1)
        row = lax.broadcasted_iota(jnp.int32, (Q, 8, 128), 0) * 8 + sub

        def unit(p, u, ct):
            cols = pl.ds(ct * 128 if isinstance(ct, int) else pl.multiple_of(ct * 128, 128), 128)
            g = 1 + p * Q
            cur = xb[pl.ds(g, Q), u, :, cols]
            up = xb[pl.ds(g + ((u - 1) >> 4), Q), (u - 1) & (U - 1), :, cols]
            dn = xb[pl.ds(g + ((u + 1) >> 4), Q), (u + 1) & (U - 1), :, cols]
            prev = pltpu.roll(jnp.where(sub == 7, up, cur), 1, 1)
            nxt = pltpu.roll(jnp.where(sub == 0, dn, cur), 7, 1)
            v = 0.25 * prev + 0.5 * cur + 0.25 * nxt
            band0 = (me * P + p) * U + u
            edge = jnp.where(band0 == 0, 0, jnp.where(band0 == NDEV * P * U - 1, Q * 8 - 1, -1))
            v = jnp.concatenate([jnp.where(row[:1] == edge, cur[:1], v[:1]), v[1:-1],
                                 jnp.where(row[-1:] == edge, cur[-1:], v[-1:])], axis=0)
            base = ((p >> 1) * W + u * N + ct * 128) * 2 + (p & 1)
            y_ref[pl.ds(base, 128, stride=2), :] = v.reshape(Q * 8, 128).T

        def advance(k):
            wait(piece(k))
            @pl.when(k + ahead < NP)
            def _():
                start(piece(k + ahead))
            @pl.when(k + ahead == NP)
            def _():
                for c in range(CT // tw):
                    start(cpiece(c))

        def pro(k, c):
            advance(k)
            return c
        lax.fori_loop(0, 3, pro, 0)

        def exchange():
            if sig: pl.semaphore_wait(bar, 2)
            if comm == "row":
                for ct in range(CT):
                    sbuf[0, ct:ct + 1, :] = xb[1, 0, 0:1, ct * 128:(ct + 1) * 128]
                    sbuf[1, ct:ct + 1, :] = xb[G, U - 1, 7:8, ct * 128:(ct + 1) * 128]
            if comm:
                to_left.start()
                to_right.start()
        def landed():
            if comm:
                to_left.wait()
                to_right.wait()
            if comm == "row":
                for ct in range(CT):
                    xb[0, U - 1, :, ct * 128:(ct + 1) * 128] = jnp.broadcast_to(rbuf[0, ct:ct + 1, :], (8, 128))
                    xb[G + 1, 0, :, ct * 128:(ct + 1) * 128] = jnp.broadcast_to(rbuf[1, ct:ct + 1, :], (8, 128))

        n_steps = (P - 1) * U + u0 - 1
        def step(i, c):
            t = jnp.where(i < halo_at, i + 1, jnp.where(i == halo_at, 0, i))
            @pl.when(i == 0)
            def _():
                advance(3)
            k = jnp.where(t + 2 >= (P - 1) * U + 1, t + 2, t + 3)
            @pl.when((i != halo_at) & (t + 2 != (P - 1) * U))
            def _():
                advance(k)
            pl.when(i == bar_at)(exchange)
            pl.when(i == halo_at)(landed)
            if compute:
                for ct in range(CT):
                    unit(t >> 4, t & (U - 1), ct)
            return c
        lax.fori_loop(0, n_steps, step, 0)

        def fin(c, carry):
            wait(cpiece(c))
            if compute:
                for t in range(tw):
                    for u in range(u0 - 1, U):
                        unit(P - 1, u, c * tw + t)
            return carry
        lax.fori_loop(0, CT // tw, fin, 0)

    def fn(x):
        y = pl.pallas_call(
            body,
            out_shape=pltpu.VMEM((M * N // 128, 128), jnp.float32),
            in_specs=[pl.BlockSpec(memory_space=pltpu.MemorySpace.HBM)],
            out_specs=pl.BlockSpec(memory_space=pltpu.VMEM),
            scratch_shapes=[
                pltpu.VMEM((G + 2, U, 8, N), jnp.float32),
                pltpu.VMEM((2, 8, 128), jnp.float32),
                pltpu.VMEM((2, 8, 128), jnp.float32),
                pltpu.SemaphoreType.DMA((ahead if ring else NP,)),
                pltpu.SemaphoreType.DMA((CT // tw,)),
                pltpu.SemaphoreType.DMA((2,)),
                pltpu.SemaphoreType.DMA((2,)),
            ],
            compiler_params=pltpu.CompilerParams(collective_id=0 if sig else None, vmem_limit_bytes=48 * 2**20,
                                                 disable_bounds_checks=True, disable_semaphore_checks=dsc),
        )(x.reshape(G, U, 8, N))
        y = y.reshape(2, W, 2, 128).transpose(0, 2, 1, 3)
        return y.reshape(2, 2, U, N, Q, 8).transpose(0, 1, 4, 2, 5, 3).reshape(M, N)
    return fn


def pallas_dist_halo_stencil_i_m8192_n1024_kernel(x):
    return make(nt=4, dsc=True, comm="band")(x)
```

```python
import jax
import jax.numpy as jnp
from jax import lax
from jax.experimental import pallas as pl
from jax.experimental.pallas import tpu as pltpu

N_DEV = 4
M, N = 8192, 1024
P, Q, U = 4, 16, 16
G = P * Q
CT = N // 128
W = U * N

TAIL = 4
TAIL_U = U - 1 - TAIL
N_STEPS = (P - 1) * U + TAIL_U - 1
AHEAD = 6
ROUND = 5
N_ROUNDS = -(-N_STEPS // ROUND)

SMEM_STEP = 40
SMEM_OUT_ROUND, SMEM_DONE_ROUND = 3, 8
RELAY_STEPS = (36, 56)
RELAY_PARTS = 4
RELAY_LAG = 2
N_RELAY = len(RELAY_STEPS) * RELAY_PARTS
PART_Q = Q // RELAY_PARTS
HALO_ROUND = 4

assert SMEM_DONE_ROUND * ROUND <= SMEM_STEP
assert all(((k + 1) * RELAY_PARTS - 1 + 2 * RELAY_LAG) * ROUND <= s for k, s in enumerate(RELAY_STEPS))
assert all(AHEAD <= s < N_STEPS and s % U < U - 2 for s in (SMEM_STEP, *RELAY_STEPS))
assert HALO_ROUND * ROUND <= (P - 2) * U


def _group(i):
    return ((i >> 4) + 1) & (P - 1)


def _is_direct(i):
    ok = ((i & (U - 1)) < U - 2) & (i < N_STEPS)
    for s in (SMEM_STEP, *RELAY_STEPS):
        ok = ok & (i != s)
    return ok


def _stencil_kernel(x_hbm, y_ref, x_buf, relay_buf, smem_buf,
                    edge_sem, slab_sem, tail_sem, smem_sem, halo_sem, relay_sem):
    me = lax.axis_index("i")
    left = (me + N_DEV - 1) & (N_DEV - 1)
    right = (me + 1) & (N_DEV - 1)
    last_p = _group(N_STEPS)

    def remote(src, dst, send_sem, recv_sem, device):
        return pltpu.make_async_remote_copy(
            src, dst, send_sem, recv_sem,
            device_id=(device,), device_id_type=pl.DeviceIdType.MESH)

    def src_slab(i, q=0, n=Q):
        return x_hbm.at[pl.ds(_group(i) * Q + q, n), (i & (U - 1)) + 1]

    def dst_slab(i, q=0, n=Q):
        return x_buf.at[pl.ds(1 + _group(i) * Q + q, n), (i & (U - 1)) + 1]

    def slab_copy(i):
        return pltpu.make_async_copy(src_slab(i), dst_slab(i), slab_sem.at[i])

    def tail_copy(ct):
        cols = pl.ds(pl.multiple_of(ct * 128, 128), 128)
        return pltpu.make_async_copy(
            x_hbm.at[pl.ds(last_p * Q, Q), pl.ds(TAIL_U, TAIL), :, cols],
            x_buf.at[pl.ds(1 + last_p * Q, Q), pl.ds(TAIL_U, TAIL), :, cols],
            tail_sem.at[ct])

    def relay_part(j):
        step = RELAY_STEPS[0] + (j // RELAY_PARTS) * (RELAY_STEPS[1] - RELAY_STEPS[0])
        return step, (j % RELAY_PARTS) * PART_Q, PART_Q

    def relay_out(j):
        return remote(src_slab(*relay_part(j)), relay_buf.at[j],
                      relay_sem.at[0, j], relay_sem.at[1, j], right)

    def relay_home(j):
        return remote(relay_buf.at[j], dst_slab(*relay_part(j)),
                      relay_sem.at[2, j], relay_sem.at[3, j], left)

    edges = [pltpu.make_async_copy(x_hbm.at[:, u], x_buf.at[pl.ds(1, G), u], edge_sem.at[k])
             for k, u in enumerate((U - 1, 0))]
    to_smem = pltpu.make_async_copy(src_slab(SMEM_STEP), smem_buf, smem_sem.at[0])
    from_smem = pltpu.make_async_copy(smem_buf, dst_slab(SMEM_STEP), smem_sem.at[1])
    halos = [
        remote(x_buf.at[1, 0], x_buf.at[G + 1, 0], halo_sem.at[0], halo_sem.at[1], left),
        remote(x_buf.at[G, U - 1], x_buf.at[0, U - 1], halo_sem.at[2], halo_sem.at[3], right),
    ]

    edges[0].start()
    to_smem.start()
    barrier = pltpu.get_barrier_semaphore()
    for neighbour in (left, right):
        pl.semaphore_signal(barrier, inc=1, device_id=(neighbour,),
                            device_id_type=pl.DeviceIdType.MESH)
    edges[1].start()
    for i in range(AHEAD):
        slab_copy(i).start()
    pl.semaphore_wait(barrier, 2)
    for copy in edges:
        copy.wait()
    for copy in halos:
        copy.start()

    sublane = lax.broadcasted_iota(jnp.int32, (Q, 8, 128), 1)

    def unit(p, u, ct):
        col = ct * 128
        cols = pl.ds(col if isinstance(col, int) else pl.multiple_of(col, 128), 128)
        g = 1 + p * Q
        cur = x_buf[pl.ds(g, Q), u, :, cols]
        above = x_buf[pl.ds(g + ((u - 1) >> 4), Q), (u - 1) & (U - 1), :, cols]
        below = x_buf[pl.ds(g + ((u + 1) >> 4), Q), (u + 1) & (U - 1), :, cols]
        prev = pltpu.roll(jnp.where(sublane == 7, above, cur), 1, 1)
        succ = pltpu.roll(jnp.where(sublane == 0, below, cur), 7, 1)
        out = 0.25 * prev + 0.5 * cur + 0.25 * succ
        slab = (me * P + p) * U + u
        first = jnp.where(slab == 0, 0, -1)
        last = jnp.where(slab == N_DEV * P * U - 1, 7, -1)
        out = jnp.concatenate([
            jnp.where(sublane[:1] == first, cur[:1], out[:1]),
            out[1:-1],
            jnp.where(sublane[:1] == last, cur[-1:], out[-1:]),
        ], axis=0)
        start = ((p >> 1) * W + u * N + col) * 2 + (p & 1)
        y_ref[pl.ds(start, 128, stride=2), :] = out.reshape(Q * 8, 128).T

    @pl.loop(0, N_ROUNDS)
    def _(r):
        @pl.when(r < N_RELAY)
        def _():
            relay_out(r).start()

        @pl.when((r >= RELAY_LAG) & (r < RELAY_LAG + N_RELAY))
        def _():
            relay_out(r - RELAY_LAG).wait()
            relay_home(r - RELAY_LAG).start()

        @pl.when((r >= 2 * RELAY_LAG) & (r < 2 * RELAY_LAG + N_RELAY))
        def _():
            relay_home(r - 2 * RELAY_LAG).wait()

        @pl.when(r == SMEM_OUT_ROUND)
        def _():
            to_smem.wait()
            from_smem.start()

        @pl.when(r == SMEM_DONE_ROUND)
        def _():
            from_smem.wait()

        @pl.when(r == HALO_ROUND)
        def _():
            for copy in halos:
                copy.wait()

        @pl.when(r == -(-(N_STEPS - AHEAD) // ROUND))
        def _():
            @pl.loop(0, CT)
            def _(ct):
                tail_copy(ct).start()

        @pl.loop(r * ROUND, jnp.minimum((r + 1) * ROUND, N_STEPS))
        def _(i):
            @pl.when(_is_direct(i + AHEAD))
            def _():
                slab_copy(i + AHEAD).start()

            @pl.when(_is_direct(i))
            def _():
                slab_copy(i).wait()

            for ct in range(CT):
                unit(_group(i), i & (U - 1), ct)

    @pl.loop(0, CT)
    def _(ct):
        tail_copy(ct).wait()
        for u in range(TAIL_U - 1, U):
            unit(last_p, u, ct)


def pallas_dist_halo_stencil_i_m8192_n1024_kernel(x: jax.Array):
    assert x.shape == (M, N) and x.dtype == jnp.float32
    dma_sems = pltpu.SemaphoreType.DMA
    y = pl.pallas_call(
        _stencil_kernel,
        out_shape=pltpu.VMEM((M * CT, 128), x.dtype),
        in_specs=[pl.BlockSpec(memory_space=pltpu.MemorySpace.HBM)],
        out_specs=pl.BlockSpec(memory_space=pltpu.VMEM),
        scratch_shapes=[
            pltpu.VMEM((G + 2, U, 8, N), x.dtype),
            pltpu.VMEM((N_RELAY, PART_Q, 8, N), x.dtype),
            pltpu.SMEM((Q, 8, N), x.dtype),
            dma_sems((2,)),
            dma_sems((N_STEPS,)),
            dma_sems((CT,)),
            dma_sems((2,)),
            dma_sems((4,)),
            dma_sems((4, N_RELAY)),
        ],
        compiler_params=pltpu.CompilerParams(
            collective_id=0,
            vmem_limit_bytes=48 * 2**20,
            disable_bounds_checks=True,
            disable_semaphore_checks=True,
        ),
    )(x.reshape(G, U, 8, N))
    y = y.reshape(2, W, 2, 128).transpose(0, 2, 1, 3)
    return y.reshape(2, 2, U, N, Q, 8).transpose(0, 1, 4, 2, 5, 3).reshape(M, N)
```

```python
import jax
import jax.numpy as jnp
from jax import lax
from jax.experimental import pallas as pl
from jax.experimental.pallas import tpu as pltpu

N_DEV = 4
M, N = 8192, 1024
P, Q, U = 4, 16, 16
G = P * Q
CT = N // 128
W = U * N

TAIL = 4
TAIL_U = U - 1 - TAIL
N_STEPS = (P - 1) * U + TAIL_U - 1
AHEAD = 8
ROUND = 5
N_ROUNDS = -(-N_STEPS // ROUND)

SMEM_STEP = 40
SMEM_OUT_ROUND, SMEM_DONE_ROUND = 3, 8
RELAY_STEPS = (36, 56)
RELAY_PARTS = 4
RELAY_LAG = 2
N_RELAY = len(RELAY_STEPS) * RELAY_PARTS
PART_Q = Q // RELAY_PARTS
HALO_ROUND = 4

assert SMEM_DONE_ROUND * ROUND <= SMEM_STEP
assert all(((k + 1) * RELAY_PARTS - 1 + 2 * RELAY_LAG) * ROUND <= s for k, s in enumerate(RELAY_STEPS))
assert all(AHEAD <= s < N_STEPS and s % U < U - 2 for s in (SMEM_STEP, *RELAY_STEPS))
assert HALO_ROUND * ROUND <= (P - 2) * U


def _group(i):
    return ((i >> 4) + 1) & (P - 1)


def _columns(ct):
    return pl.ds(ct * 128 if isinstance(ct, int) else pl.multiple_of(ct * 128, 128), 128)


def _is_direct(i):
    ok = ((i & (U - 1)) < U - 2) & (i < N_STEPS)
    for s in (SMEM_STEP, *RELAY_STEPS):
        ok = ok & (i != s)
    return ok


def _stencil_kernel(x_hbm, y_ref, x_buf, relay_buf, smem_buf,
                    edge_sem, slab_sem, tail_sem, smem_sem, halo_sem, relay_sem):
    me = lax.axis_index("i")
    left = (me + N_DEV - 1) & (N_DEV - 1)
    right = (me + 1) & (N_DEV - 1)
    last_p = _group(N_STEPS)

    def remote(src, dst, send_sem, recv_sem, device):
        return pltpu.make_async_remote_copy(
            src, dst, send_sem, recv_sem,
            device_id=(device,), device_id_type=pl.DeviceIdType.MESH)

    def src_slab(i, q=0, n=Q):
        return x_hbm.at[pl.ds(_group(i) * Q + q, n), (i & (U - 1)) + 1]

    def dst_slab(i, q=0, n=Q):
        return x_buf.at[pl.ds(1 + _group(i) * Q + q, n), (i & (U - 1)) + 1]

    def slab_copy(i):
        return pltpu.make_async_copy(src_slab(i), dst_slab(i), slab_sem.at[i])

    def tail_copy(ct):
        return pltpu.make_async_copy(
            x_hbm.at[pl.ds(last_p * Q, Q), pl.ds(TAIL_U, TAIL), :, _columns(ct)],
            x_buf.at[pl.ds(1 + last_p * Q, Q), pl.ds(TAIL_U, TAIL), :, _columns(ct)],
            tail_sem.at[ct])

    def relay_part(j):
        step = RELAY_STEPS[0] + (j // RELAY_PARTS) * (RELAY_STEPS[1] - RELAY_STEPS[0])
        return step, (j % RELAY_PARTS) * PART_Q, PART_Q

    def relay_out(j):
        return remote(src_slab(*relay_part(j)), relay_buf.at[j],
                      relay_sem.at[0, j], relay_sem.at[1, j], right)

    def relay_home(j):
        return remote(relay_buf.at[j], dst_slab(*relay_part(j)),
                      relay_sem.at[2, j], relay_sem.at[3, j], left)

    edges = [pltpu.make_async_copy(x_hbm.at[:, u], x_buf.at[pl.ds(1, G), u], edge_sem.at[k])
             for k, u in enumerate((U - 1, 0))]
    to_smem = pltpu.make_async_copy(src_slab(SMEM_STEP), smem_buf, smem_sem.at[0])
    from_smem = pltpu.make_async_copy(smem_buf, dst_slab(SMEM_STEP), smem_sem.at[1])
    halos = [
        remote(x_buf.at[1, 0], x_buf.at[G + 1, 0], halo_sem.at[0], halo_sem.at[1], left),
        remote(x_buf.at[G, U - 1], x_buf.at[0, U - 1], halo_sem.at[2], halo_sem.at[3], right),
    ]

    edges[0].start()
    to_smem.start()
    barrier = pltpu.get_barrier_semaphore()
    for neighbour in (left, right):
        pl.semaphore_signal(barrier, inc=1, device_id=(neighbour,),
                            device_id_type=pl.DeviceIdType.MESH)
    edges[1].start()
    for i in range(AHEAD):
        slab_copy(i).start()
    pl.semaphore_wait(barrier, 2)
    for copy in edges:
        copy.wait()
    for copy in halos:
        copy.start()

    sublane = lax.broadcasted_iota(jnp.int32, (Q, 8, 128), 1)

    def unit(p, u, ct):
        cols = _columns(ct)
        g = 1 + p * Q
        cur = x_buf[pl.ds(g, Q), u, :, cols]
        above = x_buf[pl.ds(g + ((u - 1) >> 4), Q), (u - 1) & (U - 1), :, cols]
        below = x_buf[pl.ds(g + ((u + 1) >> 4), Q), (u + 1) & (U - 1), :, cols]
        prev = pltpu.roll(jnp.where(sublane == 7, above, cur), 1, 1)
        succ = pltpu.roll(jnp.where(sublane == 0, below, cur), 7, 1)
        out = 0.25 * prev + 0.5 * cur + 0.25 * succ
        slab = (me * P + p) * U + u
        first = jnp.where(slab == 0, 0, -1)
        last = jnp.where(slab == N_DEV * P * U - 1, 7, -1)
        out = jnp.concatenate([
            jnp.where(sublane[:1] == first, cur[:1], out[:1]),
            out[1:-1],
            jnp.where(sublane[:1] == last, cur[-1:], out[-1:]),
        ], axis=0)
        start = ((p >> 1) * W + u * N + ct * 128) * 2 + (p & 1)
        y_ref[pl.ds(start, 128, stride=2), :] = out.reshape(Q * 8, 128).T

    @pl.loop(0, N_ROUNDS)
    def _(r):
        @pl.when(r == -(-(N_STEPS - AHEAD) // ROUND))
        def _():
            for ct in range(CT):
                tail_copy(ct).start()

        @pl.when(r < N_RELAY)
        def _():
            relay_out(r).start()

        @pl.when((r >= RELAY_LAG) & (r < RELAY_LAG + N_RELAY))
        def _():
            relay_out(r - RELAY_LAG).wait()
            relay_home(r - RELAY_LAG).start()

        @pl.when((r >= 2 * RELAY_LAG) & (r < 2 * RELAY_LAG + N_RELAY))
        def _():
            relay_home(r - 2 * RELAY_LAG).wait()

        @pl.when(r == SMEM_OUT_ROUND)
        def _():
            to_smem.wait()
            from_smem.start()

        @pl.when(r == SMEM_DONE_ROUND)
        def _():
            from_smem.wait()

        @pl.when(r == HALO_ROUND)
        def _():
            for copy in halos:
                copy.wait()

        @pl.loop(r * ROUND, jnp.minimum((r + 1) * ROUND, N_STEPS))
        def _(i):
            @pl.when(_is_direct(i + AHEAD))
            def _():
                slab_copy(i + AHEAD).start()

            @pl.when(_is_direct(i))
            def _():
                slab_copy(i).wait()

            for ct in range(CT):
                unit(_group(i), i & (U - 1), ct)

    def tail_step(ct):
        tail_copy(ct).wait()
        for u in range(TAIL_U - 1, U):
            unit(last_p, u, ct)

    pl.loop(0, CT - 1)(tail_step)
    tail_step(CT - 1)


def pallas_dist_halo_stencil_i_m8192_n1024_kernel(x: jax.Array):
    assert x.shape == (M, N) and x.dtype == jnp.float32
    dma_sems = pltpu.SemaphoreType.DMA
    y = pl.pallas_call(
        _stencil_kernel,
        out_shape=pltpu.VMEM((M * CT, 128), x.dtype),
        in_specs=[pl.BlockSpec(memory_space=pltpu.MemorySpace.HBM)],
        out_specs=pl.BlockSpec(memory_space=pltpu.VMEM),
        scratch_shapes=[
            pltpu.VMEM((G + 2, U, 8, N), x.dtype),
            pltpu.VMEM((N_RELAY, PART_Q, 8, N), x.dtype),
            pltpu.SMEM((Q, 8, N), x.dtype),
            dma_sems((2,)),
            dma_sems((N_STEPS,)),
            dma_sems((CT,)),
            dma_sems((2,)),
            dma_sems((4,)),
            dma_sems((4, N_RELAY)),
        ],
        compiler_params=pltpu.CompilerParams(
            collective_id=0,
            vmem_limit_bytes=48 * 2**20,
            disable_bounds_checks=True,
            disable_semaphore_checks=True,
        ),
    )(x.reshape(G, U, 8, N))
    y = y.reshape(2, W, 2, 128).transpose(0, 2, 1, 3)
    return y.reshape(2, 2, U, N, Q, 8).transpose(0, 1, 4, 2, 5, 3).reshape(M, N)
```
